```python
import numpy as np

kernel_name = "dist_moe_cap_ep_outshard_n2048_d512_e8_h1024"

def setup_inputs():
    x = np.random.randn(2048, 512).astype(np.float32)
    router_W = np.random.randn(512, 32).astype(np.float32) * 0.1
    scores64 = x.astype(np.float64) @ router_W.astype(np.float64)
    route_idx = np.argsort(-scores64, axis=-1)[:, :1].astype(np.int32)
    expert_W = np.random.randn(32, 512, 1024).astype(np.float32) * 0.02
    return {"x": x, "router_W": router_W, "route_idx": route_idx, "expert_W": expert_W}

def reference(x, router_W, route_idx, expert_W):
    counts = np.zeros(32, dtype=np.int64)
    out = np.zeros((2048, 1024), dtype=np.float32)
    for i in range(2048):
        e = int(route_idx[i, 0])
        if counts[e] < 51:
            out[i] = x[i] @ expert_W[e]
            counts[e] += 1
    return out
```

```python
import jax
import jax.numpy as jnp
from jax import lax
from jax.experimental import pallas as pl
from jax.experimental.pallas import tpu as pltpu

NB, E, CAP = 16, 32, 51
SL = 80
PS = 64
NDEV = 4
CH = 8
NCH = 7
EB = 6
KA = 768
KB = 512
KR = KA + KB
XG_ROWS = 8 * SL + 8 * PS
LEAD = 3
P0 = 4


def _routing(route, me):
    f32, bf16, i32 = jnp.float32, jnp.bfloat16, jnp.int32
    e_iota = lax.broadcasted_iota(i32, (NB, E, 128), 1)
    oh = route[:, None, :] == e_iota
    ohf = jnp.where(oh, 1.0, 0.0).astype(bf16).reshape(NB * E, 128)
    r = lax.broadcasted_iota(i32, (128, 256), 0)
    c = lax.broadcasted_iota(i32, (128, 256), 1)
    rhs = jnp.where((c >= 128) | (r < c), 1.0, 0.0).astype(bf16)
    pt = jnp.dot(ohf, rhs, preferred_element_type=f32)
    pin = pt[:, :128].reshape(NB, E, 128)
    tot = pt[:, 128:].reshape(NB, E, 128)
    offs = [jnp.zeros((E, 128), f32)]
    for b in range(NB):
        offs.append(offs[-1] + tot[b])
    Cd = [jnp.minimum(offs[4 * d], float(CAP)) for d in range(5)]
    ncd = [jnp.floor((Cd[d + 1] - Cd[d] + (CH - 1.0)) * (1.0 / CH)) for d in range(4)]
    npd = [n * CH for n in ncd]
    aoff = [jnp.zeros((E, 128), f32)]
    for d in range(3):
        aoff.append(aoff[-1] + npd[d])
    lane = lax.broadcasted_iota(i32, (E, 128), 1)
    erow = lax.broadcasted_iota(i32, (E, 128), 0)
    late = (erow & 7) >= EB
    nplane = jnp.zeros((E, 128), f32)
    for d in range(4):
        nplane = jnp.where(lane == 8 + d, npd[d], nplane)
    lr = lax.broadcasted_iota(i32, (E, E), 0)
    lc = lax.broadcasted_iota(i32, (E, E), 1)
    prec = jnp.where((lc < lr) & (((lr & 7) >= EB) == ((lc & 7) >= EB)), 1.0, 0.0).astype(bf16)
    tab = jnp.dot(prec, nplane.astype(bf16), preferred_element_type=f32)
    tab = tab + jnp.where(late, float(KA), 0.0)
    rme = jnp.sum(jnp.where(lane == 8 + me, tab, 0.0), axis=1, keepdims=True)

    def total(mask):
        v = jnp.sum(jnp.where(mask, nplane, 0.0), axis=1, keepdims=True)
        return jnp.sum(v, axis=0, keepdims=True) * (1.0 / CH)

    to_me = lane == 8 + me
    from_me = ((erow >> 3) == me) & (lane >= 8) & (lane < 12) & (lane != 8 + me)
    totals = [total(to_me & ~late), total(to_me & late), total(from_me & ~late), total(from_me & late)]
    for d in range(5):
        tab = jnp.where(lane == d, Cd[d], tab)
    for d in range(4):
        tab = jnp.where(lane == 16 + d, aoff[d], tab)
        tab = jnp.where(lane == 20 + d, ncd[d], tab)
        tab = jnp.where(lane == 24 + d, totals[d], tab)
    cme = jnp.sum(jnp.where(lane == me, tab, 0.0), axis=1, keepdims=True)
    kbase = rme - cme
    pos_l, slot_l, k_l = [], [], []
    for b in range(NB):
        pf = pin[b] + offs[b]
        m = oh[b]
        pos_l.append(jnp.sum(jnp.where(m, pf, 0.0), axis=0, keepdims=True))
        slot_l.append(jnp.sum(jnp.where(m, pf + (aoff[b // 4] - Cd[b // 4]), 0.0), axis=0, keepdims=True))
        k_l.append(jnp.sum(jnp.where(m, pf + kbase, 0.0), axis=0, keepdims=True))
    pos = jnp.concatenate(pos_l, axis=0)
    slotp = jnp.concatenate(slot_l, axis=0)
    kfull = jnp.concatenate(k_l, axis=0)
    keep = pos < CAP
    kpos = jnp.where(keep, kfull, -1.0)
    brow = lax.broadcasted_iota(i32, (NB, 128), 0)
    eye = lax.broadcasted_iota(i32, (128, 128), 0) == lax.broadcasted_iota(i32, (128, 128), 1)
    kiota = lax.broadcasted_iota(i32, (128, KR), 1).astype(f32)
    Rs = []
    for i in range(4):
        row = jnp.sum(jnp.where(brow == 4 * me + i, kpos, 0.0), axis=0, keepdims=True)
        col = jnp.sum(jnp.where(eye, row, 0.0), axis=1, keepdims=True)
        Rs.append(jnp.where(col == kiota, 1.0, 0.0).astype(bf16))
    R = jnp.concatenate(Rs, axis=0)
    mine = keep & ((route >> 3) == me)
    pid = jnp.where(mine, (route & 7) * PS + pos.astype(i32), -1)
    siota = lax.broadcasted_iota(i32, (8 * PS, 128), 0)
    jio = lax.broadcasted_iota(i32, (8 * PS, 128), 1).astype(f32)
    hi = jnp.zeros((8 * PS, 128), f32)
    lo = jnp.zeros((8 * PS, 128), f32)
    sl = jnp.zeros((8 * PS, 128), f32)
    for b in range(NB):
        m = pid[b:b + 1, :] == siota
        hi = jnp.where(m, float(b), hi)
        lo = jnp.where(m, jio, lo)
        sl = jnp.where(m, slotp[b:b + 1, :] + 1.0, sl)
    ones = jnp.ones((8, 128), bf16)
    dn = (((1,), (1,)), ((), ()))
    th = lax.dot_general(ones, hi.astype(bf16), dn, preferred_element_type=f32)
    tl = lax.dot_general(ones, lo.astype(bf16), dn, preferred_element_type=f32)
    ts = lax.dot_general(ones, sl.astype(bf16), dn, preferred_element_type=f32)
    tok = (th * 128.0 + tl).astype(i32)
    pio = lax.broadcasted_iota(i32, (8, 8 * PS), 1)
    tsi = ts.astype(i32)
    dst = jnp.where(tsi > 0, (pio >> 6) * SL + tsi - 1, 8 * SL + pio)
    row0 = lax.broadcasted_iota(i32, (8, 8 * PS), 0) == 0
    gt = jnp.where(row0, tok, dst)
    return tab.astype(i32), gt, R


def _compiler_params():
    base = dict(vmem_limit_bytes=100 * 1024 * 1024, collective_id=0)
    try:
        return pltpu.CompilerParams(disable_semaphore_checks=True, **base)
    except TypeError:
        return pltpu.CompilerParams(**base)


def pallas_dist_moe_cap_ep_outshard_n2048_d512_e8_h1024_kernel(
    x: jax.Array,
    router_W: jax.Array,
    route_idx: jax.Array,
    expert_W: jax.Array,
):
    del router_W
    f32, bf16, i32, u32 = jnp.float32, jnp.bfloat16, jnp.int32, jnp.uint32

    def body(route_hbm, x_hbm, w_hbm, out_ref,
             route_v, wbuf, xg, sendbuf, recvbuf, rbuf, tab_v, tok_v, tab_s, tok_s,
             w_sems, g_sems, m_sems, send_sems, recv_sems, done_sem):
        me = lax.axis_index("i")
        dk = [(me + k) % NDEV for k in range(NDEV)]

        def w_copy(i):
            h, e = i // 8, i % 8
            return pltpu.make_async_copy(w_hbm.at[e, :, pl.ds(h * 512, 512)], wbuf.at[h, e], w_sems.at[i])

        rcp = pltpu.make_async_copy(route_hbm, route_v, m_sems.at[0])
        rcp.start()
        rcp.wait()
        for i in range(LEAD):
            w_copy(i).start()

        recvbuf[...] = jnp.zeros_like(recvbuf)
        xg[0:8 * SL, :] = jnp.zeros((8 * SL, 512), f32)
        bar = pltpu.get_barrier_semaphore()
        for k in range(1, NDEV):
            pl.semaphore_signal(bar, inc=1, device_id=(dk[k],), device_id_type=pl.DeviceIdType.MESH)

        tab, gt, R = _routing(route_v[...], me)
        tab_v[...] = tab
        tok_v[...] = gt
        c2 = pltpu.make_async_copy(tok_v, tok_s, m_sems.at[2])
        c2.start()
        c1 = pltpu.make_async_copy(tab_v, tab_s, m_sems.at[1])
        c1.start()
        rbuf[...] = R
        c2.wait()
        c1.wait()

        def tree(n, lo, hi, fn):
            if lo == hi:
                if lo > 0:
                    fn(lo)
                return
            mid = (lo + hi) // 2
            lax.cond(n <= mid, lambda: tree(n, lo, mid, fn), lambda: tree(n, mid + 1, hi, fn))

        def gather(e):
            for p in range(CAP):
                t = tok_s[0, e * PS + p]
                s = tok_s[1, e * PS + p]
                pltpu.make_async_copy(x_hbm.at[pl.ds(t, 1), :], xg.at[pl.ds(s, 1), :], g_sems.at[e]).start()

        def gather_wait(e):
            pltpu.make_async_copy(xg.at[pl.ds(e * SL, 48)], xg.at[pl.ds(e * SL, 48)], g_sems.at[e]).wait()
            for p in range(48, CAP):
                pltpu.make_async_copy(xg.at[pl.ds(e * SL + p, 1)], xg.at[pl.ds(e * SL + p, 1)], g_sems.at[e]).wait()

        def piece(h, e):
            w_copy(h * 8 + e).wait()
            xe = xg[e * SL:(e + 1) * SL, :].astype(bf16)
            y = jnp.dot(xe, wbuf[h, e].astype(bf16), preferred_element_type=f32)
            ya = pltpu.bitcast(y[:, :256].astype(bf16).astype(f32), u32)
            yb = pltpu.bitcast(y[:, 256:].astype(bf16).astype(f32), u32)
            sendbuf[h, e * SL:(e + 1) * SL, :] = (ya >> 16) | (yb & jnp.uint32(0xFFFF0000))
            ph = 1 if e >= EB else 0
            eg = me * 8 + e
            for k in (1, 2, 3, 0):
                d = dk[k]
                n = tab_s[eg, 20 + d]
                ao = pl.multiple_of(tab_s[eg, 16 + d] + e * SL, CH)
                ro = pl.multiple_of(tab_s[eg, 8 + d], CH)

                def snd(c, k=k, d=d, ao=ao, ro=ro):
                    src = sendbuf.at[h, pl.ds(ao, c * CH), :]
                    dst = recvbuf.at[h, pl.ds(ro, c * CH), :]
                    rs = recv_sems.at[h * 2 + ph]
                    if k == 0:
                        pltpu.make_async_copy(src, dst, rs).start()
                    else:
                        pltpu.make_async_remote_copy(src, dst, send_sems.at[h * 2 + ph], rs, device_id=(d,),
                                                     device_id_type=pl.DeviceIdType.MESH).start()
                tree(n, 0, NCH, snd)

        def recv_wait(h, ph):
            k0 = 0 if ph == 0 else KA

            def w(c):
                dst = recvbuf.at[h, pl.ds(k0, c * CH), :]
                pltpu.make_async_copy(dst, dst, recv_sems.at[h * 2 + ph]).wait()
            tree(tab_s[0, 24 + ph], 0, (KA if ph == 0 else KB) // CH, w)

        def drain(h, ph):
            def w(c):
                src = sendbuf.at[h, pl.ds(0, c * CH), :]
                pltpu.make_async_copy(src, src, send_sems.at[h * 2 + ph]).wait()
            tree(tab_s[0, 26 + ph], 0, (EB if ph == 0 else 8 - EB) * SL // CH, w)

        def unpack(p):
            a = pltpu.bitcast(p << 16, f32).astype(bf16)
            b = pltpu.bitcast(p & jnp.uint32(0xFFFF0000), f32).astype(bf16)
            return a, b

        def scatter_a(h):
            nt = (tab_s[0, 24] + 15) // 16
            for t in range(KA // 128 + 1):
                @pl.when(nt == t)
                def _(t=t):
                    if t == 0:
                        out_ref[:, h * 512:h * 512 + 512] = jnp.zeros((512, 512), f32)
                        return
                    a, b = unpack(recvbuf[h, 0:t * 128, :])
                    Rm = rbuf[:, 0:t * 128]
                    out_ref[:, h * 512:h * 512 + 256] = jnp.dot(Rm, a, preferred_element_type=f32)
                    out_ref[:, h * 512 + 256:h * 512 + 512] = jnp.dot(Rm, b, preferred_element_type=f32)

        def scatter_b(h):
            nt = (tab_s[0, 25] + 15) // 16
            for t in range(1, KB // 128 + 1):
                @pl.when(nt == t)
                def _(t=t):
                    a, b = unpack(recvbuf[h, KA:KA + t * 128, :])
                    Rm = rbuf[:, KA:KA + t * 128]
                    out_ref[:, h * 512:h * 512 + 256] += jnp.dot(Rm, a, preferred_element_type=f32)
                    out_ref[:, h * 512 + 256:h * 512 + 512] += jnp.dot(Rm, b, preferred_element_type=f32)

        gather(0)
        w_copy(LEAD).start()
        pl.semaphore_wait(bar, NDEV - 1)
        for k in range(1, NDEV):
            pl.semaphore_signal(done_sem, inc=1, device_id=(dk[k],), device_id_type=pl.DeviceIdType.MESH)

        for e in range(8):
            if e + 1 < 8:
                gather(e + 1)
                w_copy(LEAD + e + 1).start()
            else:
                for i in range(LEAD + 8, 16):
                    w_copy(i).start()
            gather_wait(e)
            piece(0, e)
        for e in range(P0):
            piece(1, e)
        recv_wait(0, 0)
        recv_wait(0, 1)
        scatter_a(0)
        scatter_b(0)
        for e in range(P0, 8):
            piece(1, e)
        drain(0, 0)
        drain(0, 1)
        pl.semaphore_wait(done_sem, NDEV - 1)
        recv_wait(1, 0)
        scatter_a(1)
        recv_wait(1, 1)
        scatter_b(1)
        drain(1, 0)
        drain(1, 1)

    return pl.pallas_call(
        body,
        out_shape=jax.ShapeDtypeStruct((512, 1024), f32),
        in_specs=[pl.BlockSpec(memory_space=pl.ANY)] * 3,
        out_specs=pl.BlockSpec(memory_space=pltpu.VMEM),
        scratch_shapes=[
            pltpu.VMEM((16, 128), i32),
            pltpu.VMEM((2, 8, 512, 512), f32),
            pltpu.VMEM((XG_ROWS, 512), f32),
            pltpu.VMEM((2, 8 * SL, 256), u32),
            pltpu.VMEM((2, KR, 256), u32),
            pltpu.VMEM((512, KR), bf16),
            pltpu.VMEM((32, 128), i32),
            pltpu.VMEM((8, 8 * PS), i32),
            pltpu.SMEM((32, 128), i32),
            pltpu.SMEM((8, 8 * PS), i32),
            pltpu.SemaphoreType.DMA((16,)),
            pltpu.SemaphoreType.DMA((8,)),
            pltpu.SemaphoreType.DMA((3,)),
            pltpu.SemaphoreType.DMA((4,)),
            pltpu.SemaphoreType.DMA((4,)),
            pltpu.SemaphoreType.REGULAR,
        ],
        compiler_params=_compiler_params(),
    )(route_idx.reshape(16, 128), x, expert_W)
```
